```python
import numpy as np

kernel_name = "dist_max_ax1_xy_m4096_n1024"

def setup_inputs():
    return {"x": np.random.randn(8192, 2048).astype(np.float32)}

def reference(x: np.ndarray) -> np.ndarray:
    return np.max(x, axis=1, keepdims=True)
```

```python
import jax
import jax.numpy as jnp
from jax import lax
from jax.experimental import pallas as pl
from jax.experimental.pallas import tpu as pltpu

_LANES = 128
_BULK = ((2560, 512), (1024, 512), (384, 384))
_TAIL = 128


def pallas_dist_max_ax1_xy_m4096_n1024_kernel(
x: jax.Array,
):
    m, n = x.shape
    sizes = [c for c, _ in _BULK] + [_TAIL]
    offs = [sum(sizes[:i]) for i in range(len(sizes))]
    nch = len(sizes)
    assert sum(sizes) == m and n % _LANES == 0

    def body(x_hbm, o_ref, buf, part, recv, in_sems, send_sems, recv_sems):
        loads = [
            pltpu.make_async_copy(
                x_hbm.at[pl.ds(offs[i], sizes[i])],
                buf.at[pl.ds(offs[i], sizes[i])],
                in_sems.at[i],
            )
            for i in range(nch)
        ]
        for c in loads:
            c.start()

        peer = (lax.axis_index("x"), 1 - lax.axis_index("y"))
        barrier = pltpu.get_barrier_semaphore()
        pl.semaphore_signal(
            barrier, 1, device_id=peer, device_id_type=pl.DeviceIdType.MESH
        )

        def colmax(r0, g):
            vs = [
                buf[pl.ds(r0, g), j * _LANES:(j + 1) * _LANES]
                for j in range(n // _LANES)
            ]
            while len(vs) > 1:
                vs = [
                    jnp.maximum(vs[2 * k], vs[2 * k + 1])
                    for k in range(len(vs) // 2)
                ]
            return vs[0]

        def group(r0, g):
            part[:, pl.ds(r0, g)] = jnp.max(colmax(r0, g).T, axis=0, keepdims=True)

        swaps = []

        def send(i):
            sl = pl.ds(offs[i], sizes[i])
            rd = pltpu.make_async_remote_copy(
                part.at[:, sl], recv.at[:, sl], send_sems.at[i], recv_sems.at[i],
                device_id=peer, device_id_type=pl.DeviceIdType.MESH,
            )
            rd.start()
            swaps.append((rd, sl))

        for i, (rows, g) in enumerate(_BULK):
            loads[i].wait()
            if rows == g:
                group(offs[i], g)
            else:
                def step(k, carry, i=i, g=g):
                    group(pl.multiple_of(offs[i] + k * g, _LANES), g)
                    return carry
                lax.fori_loop(0, rows // g, step, 0)
            if i == 0:
                pl.semaphore_wait(barrier, 1)
            send(i)

        loads[-1].wait()
        col = jnp.max(colmax(offs[-1], _TAIL), axis=1, keepdims=True)
        ri = lax.broadcasted_iota(jnp.int32, (_TAIL, _LANES), 0)
        ci = lax.broadcasted_iota(jnp.int32, (_TAIL, _LANES), 1)
        part[:, pl.ds(offs[-1], _TAIL)] = jnp.max(
            jnp.where(ri == ci, col, -jnp.inf), axis=0, keepdims=True
        )
        send(nch - 1)

        for rd, sl in swaps[:-1]:
            rd.wait_recv()
            o_ref[:, sl] = jnp.maximum(part[:, sl], recv[:, sl])
        for rd, _ in swaps:
            rd.wait_send()
        rd, sl = swaps[-1]
        rd.wait_recv()
        o_ref[:, sl] = jnp.maximum(part[:, sl], recv[:, sl])

    out = pl.pallas_call(
        body,
        out_shape=jax.ShapeDtypeStruct((1, m), x.dtype),
        in_specs=[pl.BlockSpec(memory_space=pl.ANY)],
        out_specs=pl.BlockSpec(memory_space=pltpu.VMEM),
        scratch_shapes=[
            pltpu.VMEM((m, n), x.dtype),
            pltpu.VMEM((1, m), x.dtype),
            pltpu.VMEM((1, m), x.dtype),
            pltpu.SemaphoreType.DMA((nch,)),
            pltpu.SemaphoreType.DMA((nch,)),
            pltpu.SemaphoreType.DMA((nch,)),
        ],
        compiler_params=pltpu.CompilerParams(
            vmem_limit_bytes=64 * 1024 * 1024,
            collective_id=0,
            disable_semaphore_checks=True,
            disable_bounds_checks=True,
        ),
    )(x)
    return out.reshape(m, 1)
```

```python
import jax
import jax.numpy as jnp
from jax import lax
from jax.experimental import pallas as pl
from jax.experimental.pallas import tpu as pltpu

_B = 128
_D = 8
_LAG = 6


def pallas_dist_max_ax1_xy_m4096_n1024_kernel(
x: jax.Array,
):
    m, n = x.shape
    half = m // 2
    nb = half // _B
    per = _B // _D
    assert half % _B == 0 and n % 128 == 0 and nb > _LAG
    pieces = (
        (half, m),
        (0, half - 8 * _B),
        (half - 8 * _B, half - 2 * _B),
        (half - 2 * _B, half - _B),
        (half - _B, half),
    )

    def body(x_hbm, o_ref, buf, part, recv, lo_sems, hi_sems, send_sems, recv_sems):
        def load(r0, rows, sem):
            r0 = pl.multiple_of(r0, _D)
            return pltpu.make_async_copy(
                x_hbm.at[pl.ds(r0, rows)], buf.at[pl.ds(r0, rows)], sem
            )

        def issue(j, k0, k1):
            for k in range(k0, k1):
                load(j * _B + k * _D, _D, lo_sems.at[j]).start(priority=1)
                load(half + j * _B + k * _D, _D, hi_sems.at[j]).start(priority=0)

        ri = lax.broadcasted_iota(jnp.int32, (_B, 128), 0)
        ci = lax.broadcasted_iota(jnp.int32, (_B, 128), 1)

        def reduce_block(r0, sem):
            load(r0, _B, sem).wait()
            r0 = pl.multiple_of(r0, _B)
            vs = [buf[pl.ds(r0, _B), k * 128:(k + 1) * 128] for k in range(n // 128)]
            while len(vs) > 1:
                vs = [jnp.maximum(a, b) for a, b in zip(vs[0::2], vs[1::2])] + (
                    [vs[-1]] if len(vs) % 2 else []
                )
            col = jnp.max(vs[0], axis=1, keepdims=True)
            part[:, pl.ds(r0, _B)] = jnp.max(
                jnp.where(ri == ci, col, -jnp.inf), axis=0, keepdims=True
            )

        def do_lo(j):
            reduce_block(j * _B, lo_sems.at[j])

        def do_hi(j):
            reduce_block(half + j * _B, hi_sems.at[j])

        issue(0, 0, per)

        peer = (lax.axis_index("x"), 1 - lax.axis_index("y"))
        barrier = pltpu.get_barrier_semaphore()
        pl.semaphore_signal(
            barrier, 1, device_id=peer, device_id_type=pl.DeviceIdType.MESH
        )

        def prologue(j, c):
            issue(j, 0, per)
            return c

        lax.fori_loop(1, _LAG, prologue, 0)

        def steady(j, c):
            issue(j, 0, per // 2)
            do_hi(j - _LAG)
            issue(j, per // 2, per)
            do_lo(j - _LAG)
            return c

        lax.fori_loop(_LAG, nb, steady, 0)

        def drain_hi(j, c):
            do_hi(j)
            return c

        lax.fori_loop(nb - _LAG, nb, drain_hi, 0)

        pl.semaphore_wait(barrier, 1)

        swaps = []
        lo_done = nb - _LAG
        for i, (a, b) in enumerate(pieces):
            while a < half and lo_done * _B < b:
                do_lo(lo_done)
                lo_done += 1
            sl = pl.ds(a, b - a)
            rd = pltpu.make_async_remote_copy(
                part.at[:, sl], recv.at[:, sl], send_sems.at[i], recv_sems.at[i],
                device_id=peer, device_id_type=pl.DeviceIdType.MESH,
            )
            rd.start()
            swaps.append((rd, sl))

        for rd, sl in swaps[:-1]:
            rd.wait_recv()
            o_ref[:, sl] = jnp.maximum(part[:, sl], recv[:, sl])
        for rd, _ in swaps:
            rd.wait_send()
        rd, sl = swaps[-1]
        rd.wait_recv()
        o_ref[:, sl] = jnp.maximum(part[:, sl], recv[:, sl])

    out = pl.pallas_call(
        body,
        out_shape=jax.ShapeDtypeStruct((1, m), x.dtype),
        in_specs=[pl.BlockSpec(memory_space=pl.ANY)],
        out_specs=pl.BlockSpec(memory_space=pltpu.VMEM),
        scratch_shapes=[
            pltpu.VMEM((m, n), x.dtype),
            pltpu.VMEM((1, m), x.dtype),
            pltpu.VMEM((1, m), x.dtype),
            pltpu.SemaphoreType.DMA((nb,)),
            pltpu.SemaphoreType.DMA((nb,)),
            pltpu.SemaphoreType.DMA((len(pieces),)),
            pltpu.SemaphoreType.DMA((len(pieces),)),
        ],
        compiler_params=pltpu.CompilerParams(
            vmem_limit_bytes=64 * 1024 * 1024,
            collective_id=0,
            disable_semaphore_checks=True,
            disable_bounds_checks=True,
        ),
    )(x)
    return out.reshape(m, 1)
```

```python
import jax
import jax.numpy as jnp
from jax import lax
from jax.experimental import pallas as pl
from jax.experimental.pallas import tpu as pltpu

_B = 128
_D = 8
_PER = _B // _D
_HEAD = 28
_LAG_LO = 4
_LAG_HI = 3
_TAIL = (96, 32)


def pallas_dist_max_ax1_xy_m4096_n1024_kernel(
x: jax.Array,
):
    m, n = x.shape
    nb_hi = (m // _B - 2) // 2
    nb_lo = m // _B - nb_hi
    m_lo = nb_lo * _B
    shift = 2 * _PER - _HEAD
    tail_off = [sum(_TAIL[:i]) for i in range(len(_TAIL))]
    n_swaps = 5
    assert m % _B == 0 and n % 128 == 0 and sum(_TAIL) == _B
    assert 0 <= shift < _PER and nb_hi > _LAG_LO + _LAG_HI

    def body(x_hbm, o_ref, buf, part, recv,
             lo_sems, hi_sems, tail_sems, send_sems, recv_sems):
        def load(r0, rows, sem):
            if not isinstance(r0, int):
                r0 = pl.multiple_of(r0, _D)
            return pltpu.make_async_copy(
                x_hbm.at[pl.ds(r0, rows)], buf.at[pl.ds(r0, rows)], sem
            )

        def start_lo(blk, k):
            if isinstance(blk, int) and blk == nb_lo - 1:
                t = max(q for q, off in enumerate(tail_off) if off <= k * _D)
                sem = tail_sems.at[t]
            else:
                sem = lo_sems.at[blk]
            load(blk * _B + k * _D, _D, sem).start(priority=1)

        def start_hi(blk, k):
            blk, k = blk + k // _PER, k % _PER
            load(m_lo + blk * _B + k * _D, _D, hi_sems.at[blk]).start(priority=0)

        def row_max(r0, rows, lane0):
            vs = [
                buf[pl.ds(r0, rows), k * 128:(k + 1) * 128]
                for k in range(n // 128)
            ]
            while len(vs) > 1:
                vs = [jnp.maximum(a, b) for a, b in zip(vs[0::2], vs[1::2])] + (
                    [vs[-1]] if len(vs) % 2 else []
                )
            col = jnp.max(vs[0], axis=1, keepdims=True)
            ri = lax.broadcasted_iota(jnp.int32, (rows, 128), 0) + lane0
            ci = lax.broadcasted_iota(jnp.int32, (rows, 128), 1)
            diag = jnp.where(ri == ci, col, -jnp.inf)
            return jnp.max(diag.reshape(rows // 8, 8, 128), axis=0)

        def reduce_block(r0, sem):
            load(r0, _B, sem).wait()
            if not isinstance(r0, int):
                r0 = pl.multiple_of(r0, _B)
            part[:, pl.ds(r0, _B)] = jnp.max(
                row_max(r0, _B, 0), axis=0, keepdims=True
            )

        def do_lo(blk):
            reduce_block(blk * _B, lo_sems.at[blk])

        def do_hi(blk):
            reduce_block(m_lo + blk * _B, hi_sems.at[blk])

        for i in range(3 * _PER):
            if i >= _HEAD:
                start_hi(0, i - _HEAD)
            start_lo(i // _PER, i % _PER)

        peer = (lax.axis_index("x"), 1 - lax.axis_index("y"))
        barrier = pltpu.get_barrier_semaphore()
        pl.semaphore_signal(
            barrier, 1, device_id=peer, device_id_type=pl.DeviceIdType.MESH
        )

        def step(j, carry):
            for k in range(_PER):
                start_hi(j, k + shift)
                start_lo(j + 2, k)

            @pl.when(j + 2 >= _LAG_LO)
            def _():
                do_lo(j + 2 - _LAG_LO)

            @pl.when(j >= _LAG_HI)
            def _():
                do_hi(j - _LAG_HI)

            return carry

        last = nb_hi - 1
        lax.fori_loop(1, last, step, 0)
        for k in range(_PER):
            if k + shift < _PER:
                start_hi(last, k + shift)
            start_lo(last + 2, k)
        lo_done = last + 2 - _LAG_LO
        hi_done = last - _LAG_HI

        swaps = []

        def send(a, b):
            i = len(swaps)
            sl = pl.ds(a, b - a)
            rd = pltpu.make_async_remote_copy(
                part.at[:, sl], recv.at[:, sl], send_sems.at[i], recv_sems.at[i],
                device_id=peer, device_id_type=pl.DeviceIdType.MESH,
            )
            rd.start()
            swaps.append((rd, sl))

        pl.semaphore_wait(barrier, 1)
        send(0, lo_done * _B)
        send(m_lo, m_lo + hi_done * _B)

        rest = [(2 * b, do_lo, b) for b in range(lo_done, nb_lo - 1)]
        rest += [(2 * b + 1, do_hi, b) for b in range(hi_done, nb_hi)]
        for _, fn, b in sorted(rest, key=lambda e: e[0]):
            fn(b)
            if fn is do_hi and b == last:
                send(m_lo + hi_done * _B, m)
        base = m_lo - _B
        send(lo_done * _B, base)

        acc = None
        for t, rows in enumerate(_TAIL):
            load(base + tail_off[t], rows, tail_sems.at[t]).wait()
            piece = row_max(base + tail_off[t], rows, tail_off[t])
            acc = piece if acc is None else jnp.maximum(acc, piece)
        part[:, pl.ds(base, _B)] = jnp.max(acc, axis=0, keepdims=True)
        send(base, m_lo)
        assert len(swaps) == n_swaps

        for rd, sl in swaps[:-1]:
            rd.wait_recv()
            o_ref[:, sl] = jnp.maximum(part[:, sl], recv[:, sl])
        for rd, _ in swaps:
            rd.wait_send()
        rd, sl = swaps[-1]
        rd.wait_recv()
        o_ref[:, sl] = jnp.maximum(part[:, sl], recv[:, sl])

    out = pl.pallas_call(
        body,
        out_shape=jax.ShapeDtypeStruct((1, m), x.dtype),
        in_specs=[pl.BlockSpec(memory_space=pl.ANY)],
        out_specs=pl.BlockSpec(memory_space=pltpu.VMEM),
        scratch_shapes=[
            pltpu.VMEM((m, n), x.dtype),
            pltpu.VMEM((1, m), x.dtype),
            pltpu.VMEM((1, m), x.dtype),
            pltpu.SemaphoreType.DMA((nb_lo - 1,)),
            pltpu.SemaphoreType.DMA((nb_hi,)),
            pltpu.SemaphoreType.DMA((len(_TAIL),)),
            pltpu.SemaphoreType.DMA((n_swaps,)),
            pltpu.SemaphoreType.DMA((n_swaps,)),
        ],
        compiler_params=pltpu.CompilerParams(
            vmem_limit_bytes=64 * 1024 * 1024,
            collective_id=0,
            disable_semaphore_checks=True,
            disable_bounds_checks=True,
        ),
    )(x)
    return out.reshape(m, 1)
```

```python
import jax, jax.numpy as jnp
from jax import lax
from jax.experimental import pallas as pl
from jax.experimental.pallas import tpu as pltpu

NEG = float("-inf")
B = 128

def make(P=27, tail=(12, 4), RS=2, lag=2, SH=1):
    S = 15
    R = 32
    def fn(x):
        m, n = x.shape
        CB = n // 128
        TS = R * CB
        xt = x.reshape(m // 8, 8, CB, 128).transpose(0, 2, 1, 3).reshape(m // 8 * CB, 8, 128)
        nst = R // RS
        CH = S * RS
        HP = CH // 2
        NM = (S + 1) + (R - 1) * S
        nH = NM // 2
        nLm = NM - nH
        MM = S * R * 8
        tb = [16]
        for t in tail: tb.append(tb[-1] + t)
        def body(x_hbm, o_ref, buf, part, recv, psem, sems, tsem, ssems, rsems):
            def unit(s, i, sem, prio, nt=CB):
                if isinstance(i, int) and s == 0 and i == 0:
                    c = pltpu.make_async_copy(x_hbm.at[pl.ds(0, CB - SH)], buf.at[0, pl.ds(SH, CB - SH)], sem)
                else:
                    c = pltpu.make_async_copy(x_hbm.at[pl.ds(s * TS + i * CB - SH, nt)], buf.at[s, pl.ds(i * CB, nt)], sem)
                c.start(priority=prio)
            def pos(k, prio, q=0):
                if isinstance(q, int): k, q = k + CH * q, 0
                if k < S + 1:
                    unit(k, 0, psem.at[0 if k == 0 else 1], prio); return
                j = k - (S + 1)
                dq, j = divmod(j, CH)
                qq = q + dq
                unit(j % S, qq * RS + 1 + j // S, sems.at[qq], prio)
            def tailL(t):
                i = t + 1
                g = min(z for z in range(len(tb)) if i <= tb[z])
                unit(S, i, tsem.at[g], 1, nt=CB + SH if i == R - 1 else CB)
            def L_static(i):
                if i < nLm: pos(2 * i, 1)
                elif i - nLm < R - 1: tailL(i - nLm)
            def red(v, lane0):
                G = v.shape[0] // CB
                v = jnp.max(v.reshape(G, CB, 8, 128), axis=1)
                mm = jnp.max(v, axis=2, keepdims=True)
                gi = lax.broadcasted_iota(jnp.int32, (G, 8, 128), 0)
                ri = lax.broadcasted_iota(jnp.int32, (G, 8, 128), 1)
                ci = lax.broadcasted_iota(jnp.int32, (G, 8, 128), 2)
                d = jnp.where(ci - ri - 8 * gi == lane0, mm, NEG)
                return jnp.max(d, axis=0)
            def wait(ref, sem):
                pltpu.make_async_copy(ref, ref, sem).wait()
            def comp_step(q):
                last = isinstance(q, int) and q == nst - 1
                nr = RS - 1 if last else RS
                if nr: wait(buf.at[pl.ds(0, S), pl.ds((q * RS + 1) * CB, nr * CB)], sems.at[q])
                lane0 = (q * RS * 8) % B
                blk0 = (q * RS * 8) // B * B
                for s in range(S):
                    t0 = q * RS * CB + SH
                    if last:
                        v = jnp.concatenate([buf[s, pl.ds(t0, RS * CB - SH)], buf[s + 1, pl.ds(0, SH)]], axis=0)
                    else:
                        v = buf[s, pl.ds(t0, RS * CB)]
                    c0 = s * R * 8 + blk0
                    if not isinstance(c0, int): c0 = pl.multiple_of(c0, B)
                    r = jnp.max(red(v, lane0), axis=0, keepdims=True)
                    part[:, pl.ds(c0, B)] = jnp.maximum(part[:, pl.ds(c0, B)], r)

            h0 = (S + 1) // 2
            for i in range(P): L_static(i)
            for i in range(h0 + HP * lag):
                pos(2 * i + 1, 0); L_static(i + P)
                if i == 20:
                    mx = lax.axis_index("x"); my = lax.axis_index("y")
                    peer = (mx, 1 - my)
                    bar = pltpu.get_barrier_semaphore()
                    pl.semaphore_signal(bar, 1, device_id=peer, device_id_type=pl.DeviceIdType.MESH)
                    part[...] = jnp.full(part.shape, NEG, part.dtype)
            wait(buf.at[0, pl.ds(SH, CB - SH)], psem.at[0])
            wait(buf.at[pl.ds(1, S), pl.ds(0, CB)], psem.at[1])
            qd = (NM - (S + 1) - 2 * P) // CH
            def step(q, c):
                for i in range(h0, h0 + HP):
                    pos(2 * i + 1, 0, q)
                    pos(2 * (i + P), 1, q)
                comp_step(q - lag)
                return c
            lax.fori_loop(lag, qd, step, 0)
            for q in range(qd, nst):
                for i in range(h0 + HP * q, h0 + HP * (q + 1)):
                    if i < nH: pos(2 * i + 1, 0)
                    L_static(i + P)
                comp_step(q - lag)
            assert h0 + HP * nst + P >= nLm + R - 1
            for q in range(nst - lag, nst): comp_step(q)
            rds = []
            def send(a, b):
                i = len(rds)
                sl = pl.ds(a, b - a)
                rd = pltpu.make_async_remote_copy(part.at[:, sl], recv.at[:, sl], ssems.at[i], rsems.at[i],
                        device_id=peer, device_id_type=pl.DeviceIdType.MESH)
                rd.start()
                rds.append((rd, sl))
            pl.semaphore_wait(bar, 1)
            send(0, MM)
            wait(buf.at[S, pl.ds(CB, 16 * CB)], tsem.at[0])
            part[:, pl.ds(MM, B)] = jnp.max(red(buf[S, pl.ds(SH, 16 * CB)], 0), axis=0, keepdims=True)
            send(MM, MM + B)
            base = MM + B
            d = None
            for g in range(1, len(tb)):
                a, b = tb[g - 1], tb[g]
                e = min((b + 1) * CB, TS + SH)
                wait(buf.at[S, pl.ds((a + 1) * CB, e - (a + 1) * CB)], tsem.at[g])
                di = red(buf[S, pl.ds(a * CB + SH, (b - a) * CB)], (a - 16) * 8)
                d = di if d is None else jnp.maximum(d, di)
            part[:, pl.ds(base, B)] = jnp.max(d, axis=0, keepdims=True)
            send(base, base + B)
            for rd, sl in rds[:-1]:
                rd.wait_recv()
                o_ref[:, sl] = jnp.maximum(part[:, sl], recv[:, sl])
            for rd, sl in rds:
                rd.wait_send()
            rd, sl = rds[-1]
            rd.wait_recv()
            o_ref[:, sl] = jnp.maximum(part[:, sl], recv[:, sl])
        ns = 3
        o = pl.pallas_call(body,
            in_specs=[pl.BlockSpec(memory_space=pl.ANY)],
            out_specs=pl.BlockSpec(memory_space=pltpu.VMEM),
            out_shape=jax.ShapeDtypeStruct((1, m), x.dtype),
            scratch_shapes=[pltpu.VMEM((S + 1, TS + SH, 8, 128), x.dtype), pltpu.VMEM((1, m), x.dtype), pltpu.VMEM((1, m), x.dtype),
                            pltpu.SemaphoreType.DMA((2,)), pltpu.SemaphoreType.DMA((nst,)), pltpu.SemaphoreType.DMA((len(tb),)),
                            pltpu.SemaphoreType.DMA((ns,)), pltpu.SemaphoreType.DMA((ns,))],
            compiler_params=pltpu.CompilerParams(vmem_limit_bytes=64*1024*1024, collective_id=0,
                disable_semaphore_checks=True),
            )(xt)
        return o.reshape(m, 1)
    return fn

def pallas_dist_max_ax1_xy_m4096_n1024_kernel(x):
    return make()(x)
```

```python
import jax
import jax.numpy as jnp
from jax import lax
from jax.experimental import pallas as pl
from jax.experimental.pallas import tpu as pltpu

_B = 128
_R = 32
_RS = 2
_LAG = 2
_HEAD = 27
_SH = 1
_TAIL = (16, 28, 32)


def pallas_dist_max_ax1_xy_m4096_n1024_kernel(
x: jax.Array,
):
    m, n = x.shape
    cb = n // 128
    ts = _R * cb
    ns = m // (8 * _R) - 1
    m_main = ns * _R * 8
    n_steps = _R // _RS
    chunk = ns * _RS
    pairs = chunk // 2
    n_main = (ns + 1) + (_R - 1) * ns
    n_hi = n_main // 2
    n_lo = n_main - n_hi
    h0 = (ns + 1) // 2
    assert m % (8 * _R) == 0 and n % 128 == 0 and 8 * _R == 2 * _B
    assert chunk % 2 == 0 and (ns + 1) % 2 == 0 and 0 < _SH < cb
    assert h0 + pairs * n_steps + _HEAD >= n_lo + _R - 1

    xt = x.reshape(m // 8, 8, cb, 128).transpose(0, 2, 1, 3)
    xt = xt.reshape(m // 8 * cb, 8, 128)

    def body(x_hbm, o_ref, buf, part, recv,
             head_sems, step_sems, tail_sems, send_sems, recv_sems):
        def start(s, i, sem, prio, extra=0):
            skip = _SH if (s == 0 and isinstance(i, int) and i == 0) else 0
            nt = cb + extra - skip
            pltpu.make_async_copy(
                x_hbm.at[pl.ds(s * ts + i * cb - _SH + skip, nt)],
                buf.at[s, pl.ds(i * cb + skip, nt)],
                sem,
            ).start(priority=prio)

        def start_main(k, prio, q=0):
            if isinstance(q, int):
                k, q = k + chunk * q, 0
            if k <= ns:
                start(k, 0, head_sems.at[min(k, 1)], prio)
            else:
                dq, j = divmod(k - ns - 1, chunk)
                start(j % ns, (q + dq) * _RS + 1 + j // ns,
                      step_sems.at[q + dq], prio)

        def start_lo(i):
            if i < n_lo:
                start_main(2 * i, 1)
            elif i - n_lo + 1 < _R:
                u = i - n_lo + 1
                g = min(z for z, end in enumerate(_TAIL) if u <= end)
                start(ns, u, tail_sems.at[g], 1, _SH if u == _R - 1 else 0)

        def wait(ref, sem):
            pltpu.make_async_copy(ref, ref, sem).wait()

        def row_max(tiles, lane0):
            g = tiles.shape[0] // cb
            v = jnp.max(tiles.reshape(g, cb, 8, 128), axis=1)
            col = jnp.max(v, axis=2, keepdims=True)
            gi = lax.broadcasted_iota(jnp.int32, (g, 8, 128), 0)
            ri = lax.broadcasted_iota(jnp.int32, (g, 8, 128), 1)
            ci = lax.broadcasted_iota(jnp.int32, (g, 8, 128), 2)
            diag = jnp.where(ci - ri - 8 * gi == lane0, col, -jnp.inf)
            return jnp.max(diag, axis=0)

        def reduce_step(q):
            last = isinstance(q, int) and q == n_steps - 1
            rounds = _RS - 1 if last else _RS
            wait(buf.at[pl.ds(0, ns), pl.ds((q * _RS + 1) * cb, rounds * cb)],
                 step_sems.at[q])
            row0 = q * _RS * 8
            t0 = q * _RS * cb + _SH
            for s in range(ns):
                if last:
                    tiles = jnp.concatenate(
                        [buf[s, pl.ds(t0, _RS * cb - _SH)],
                         buf[s + 1, pl.ds(0, _SH)]], axis=0)
                else:
                    tiles = buf[s, pl.ds(t0, _RS * cb)]
                c0 = s * _R * 8 + row0 // _B * _B
                if not isinstance(c0, int):
                    c0 = pl.multiple_of(c0, _B)
                new = jnp.max(row_max(tiles, row0 % _B), axis=0, keepdims=True)
                part[:, pl.ds(c0, _B)] = jnp.maximum(part[:, pl.ds(c0, _B)], new)

        for i in range(_HEAD):
            start_lo(i)
        for i in range(h0 + pairs):
            start_main(2 * i + 1, 0)
            start_lo(i + _HEAD)

        peer = (lax.axis_index("x"), 1 - lax.axis_index("y"))
        barrier = pltpu.get_barrier_semaphore()
        pl.semaphore_signal(
            barrier, 1, device_id=peer, device_id_type=pl.DeviceIdType.MESH
        )
        part[...] = jnp.full(part.shape, -jnp.inf, part.dtype)

        for i in range(h0 + pairs, h0 + pairs * _LAG):
            start_main(2 * i + 1, 0)
            start_lo(i + _HEAD)
        wait(buf.at[0, pl.ds(_SH, cb - _SH)], head_sems.at[0])
        wait(buf.at[pl.ds(1, ns), pl.ds(0, cb)], head_sems.at[1])

        def step(q, carry):
            for i in range(h0, h0 + pairs):
                start_main(2 * i + 1, 0, q)
                start_main(2 * (i + _HEAD), 1, q)
            reduce_step(q - _LAG)
            return carry

        q_loop = (n_main - ns - 1 - 2 * _HEAD) // chunk
        lax.fori_loop(_LAG, q_loop, step, 0)
        for q in range(q_loop, n_steps):
            for i in range(h0 + pairs * q, h0 + pairs * (q + 1)):
                if i < n_hi:
                    start_main(2 * i + 1, 0)
                start_lo(i + _HEAD)
            reduce_step(q - _LAG)
        for q in range(n_steps - _LAG, n_steps):
            reduce_step(q)

        swaps = []

        def send(a, b):
            i = len(swaps)
            sl = pl.ds(a, b - a)
            rd = pltpu.make_async_remote_copy(
                part.at[:, sl], recv.at[:, sl], send_sems.at[i], recv_sems.at[i],
                device_id=peer, device_id_type=pl.DeviceIdType.MESH,
            )
            rd.start()
            swaps.append((rd, sl))

        pl.semaphore_wait(barrier, 1)
        send(0, m_main)

        acc = None
        for g, (a, b) in enumerate(zip((0,) + _TAIL[:-1], _TAIL)):
            lo, hi = (a + 1) * cb, min((b + 1) * cb, ts + _SH)
            wait(buf.at[ns, pl.ds(lo, hi - lo)], tail_sems.at[g])
            piece = row_max(
                buf[ns, pl.ds(a * cb + _SH, (b - a) * cb)], a * 8 % _B
            )
            acc = piece if acc is None else jnp.maximum(acc, piece)
            if b * 8 % _B == 0:
                c0 = m_main + b * 8 - _B
                part[:, pl.ds(c0, _B)] = jnp.max(acc, axis=0, keepdims=True)
                send(c0, c0 + _B)
                acc = None

        for rd, sl in swaps[:-1]:
            rd.wait_recv()
            o_ref[:, sl] = jnp.maximum(part[:, sl], recv[:, sl])
        for rd, _ in swaps:
            rd.wait_send()
        rd, sl = swaps[-1]
        rd.wait_recv()
        o_ref[:, sl] = jnp.maximum(part[:, sl], recv[:, sl])

    out = pl.pallas_call(
        body,
        out_shape=jax.ShapeDtypeStruct((1, m), x.dtype),
        in_specs=[pl.BlockSpec(memory_space=pl.ANY)],
        out_specs=pl.BlockSpec(memory_space=pltpu.VMEM),
        scratch_shapes=[
            pltpu.VMEM((ns + 1, ts + _SH, 8, 128), x.dtype),
            pltpu.VMEM((1, m), x.dtype),
            pltpu.VMEM((1, m), x.dtype),
            pltpu.SemaphoreType.DMA((2,)),
            pltpu.SemaphoreType.DMA((n_steps,)),
            pltpu.SemaphoreType.DMA((len(_TAIL),)),
            pltpu.SemaphoreType.DMA((3,)),
            pltpu.SemaphoreType.DMA((3,)),
        ],
        compiler_params=pltpu.CompilerParams(
            vmem_limit_bytes=64 * 1024 * 1024,
            collective_id=0,
            disable_semaphore_checks=True,
        ),
    )(xt)
    return out.reshape(m, 1)
```

```python
import jax
import jax.numpy as jnp
from jax import lax
from jax.experimental import pallas as pl
from jax.experimental.pallas import tpu as pltpu

_G = 16
_R = 2 * _G
_SH = 1
_HEAD = 27
_LAG = 34
_HALVED = 13
_STEPS = (4, 8, 12, 16, 20, 24, 28, 30, 32)
_TAIL = (28, 32)


def pallas_dist_max_ax1_xy_m4096_n1024_kernel(
x: jax.Array,
):
    m, n = x.shape
    cb = n // 128
    ts = _R * cb
    ns = m // (8 * _R)
    assert m % (8 * _R) == 0 and n % 256 == 0 and 0 < _SH < cb
    assert _G in _STEPS and _STEPS[-1] == _R and _TAIL[-1] == _R

    main = [(s, i) for i in range(_R) for s in range(ns if i <= _G else ns - 1)]
    lo_main, hi_main = main[0::2], main[1::2]
    lo_tail = []
    for i in range(_G + 1, _R):
        piece = min(t for t, end in enumerate(_TAIL) if i <= end)
        nt = cb + (_SH if i == _R - 1 else 0)
        cut = cb // 2 if i >= _R - _HALVED else nt
        lo_tail.append((i * cb, cut, piece))
        if cut < nt:
            lo_tail.append((i * cb + cut, nt - cut, piece))
    n_pairs = max(len(hi_main), len(lo_main) + len(lo_tail) - _HEAD)

    def step_of(i):
        return min(q for q, end in enumerate(_STEPS) if i <= end)

    last_pair = {step_of(i): k // 2 for k, (_, i) in enumerate(main)}

    xt = x.reshape(m // 8, 8, cb, 128).transpose(0, 2, 1, 3)
    xt = xt.reshape(m // 8 * cb, 8, 128)

    def body(x_hbm, o_ref, buf, part, recv, tail_part, tail_recv,
             head_sems, step_sems, tail_sems, send_sems, recv_sems):
        def start(s, t0, nt, sem, prio):
            pltpu.make_async_copy(
                x_hbm.at[pl.ds(s * ts + t0 - _SH, nt)],
                buf.at[s, pl.ds(t0, nt)],
                sem,
            ).start(priority=prio)

        def start_main(s, i, prio):
            if i > 0:
                start(s, i * cb, cb, step_sems.at[step_of(i)], prio)
            elif s > 0:
                start(s, 0, cb, head_sems.at[1], prio)
            else:
                start(0, _SH, cb - _SH, head_sems.at[0], prio)

        def start_lo(k):
            if k < len(lo_main):
                start_main(*lo_main[k], 1)
            elif k - len(lo_main) < len(lo_tail):
                t0, nt, piece = lo_tail[k - len(lo_main)]
                start(ns - 1, t0, nt, tail_sems.at[piece], 1)

        def wait(ref, sem):
            pltpu.make_async_copy(ref, ref, sem).wait()

        def row_max(tiles, lane0):
            g = tiles.shape[0] // cb
            tiles = tiles.reshape(g, cb, 8, 128)
            vs = [tiles[:, k] for k in range(cb)]
            while len(vs) > 1:
                vs = [jnp.maximum(a, b) for a, b in zip(vs[0::2], vs[1::2])] + (
                    vs[-1:] if len(vs) % 2 else []
                )
            col = jnp.max(vs[0], axis=2, keepdims=True)
            gi = lax.broadcasted_iota(jnp.int32, (g, 8, 128), 0)
            ri = lax.broadcasted_iota(jnp.int32, (g, 8, 128), 1)
            ci = lax.broadcasted_iota(jnp.int32, (g, 8, 128), 2)
            diag = jnp.where(ci - ri - 8 * gi == lane0, col, -jnp.inf)
            return jnp.max(diag, axis=0)

        peer = (lax.axis_index("x"), 1 - lax.axis_index("y"))
        barrier = pltpu.get_barrier_semaphore()
        swaps = [
            pltpu.make_async_remote_copy(
                src, dst, send_sems.at[i], recv_sems.at[i],
                device_id=peer, device_id_type=pl.DeviceIdType.MESH,
            )
            for i, (src, dst) in enumerate([
                (part.at[0], recv.at[0]),
                (part.at[1], recv.at[1]),
                (tail_part, tail_recv),
            ])
        ]

        def reduce_step(q):
            a, b = (_STEPS[q - 1] if q else 0), _STEPS[q]
            streams = ns if b <= _G else ns - 1
            if q == 0:
                wait(buf.at[0, pl.ds(_SH, cb - _SH)], head_sems.at[0])
                wait(buf.at[pl.ds(1, ns - 1), pl.ds(0, cb)], head_sems.at[1])
            rounds = min(b, _R - 1) - a
            wait(buf.at[pl.ds(0, streams), pl.ds((a + 1) * cb, rounds * cb)],
                 step_sems.at[q])
            t0, nt = a * cb + _SH, (b - a) * cb
            for s in range(streams):
                if b == _R:
                    tiles = jnp.concatenate(
                        [buf[s, pl.ds(t0, nt - _SH)], buf[s + 1, pl.ds(0, _SH)]],
                        axis=0,
                    )
                else:
                    tiles = buf[s, pl.ds(t0, nt)]
                new = jnp.max(row_max(tiles, a % _G * 8), axis=0, keepdims=True)
                row = part.at[a // _G, pl.ds(s, 1), :]
                row[...] = jnp.maximum(row[...], new)
            if b == _G:
                pl.semaphore_wait(barrier, 1)
                swaps[0].start()
            if b == _R:
                swaps[1].start()

        for k in range(_HEAD):
            start_lo(k)
        q = 0
        for k in range(n_pairs):
            if k < len(hi_main):
                start_main(*hi_main[k], 0)
            start_lo(k + _HEAD)
            if k == 20:
                pl.semaphore_signal(
                    barrier, 1,
                    device_id=peer, device_id_type=pl.DeviceIdType.MESH,
                )
                part[...] = jnp.full(part.shape, -jnp.inf, part.dtype)
            if k >= last_pair[q] + _LAG:
                reduce_step(q)
                q += 1
        for q in range(q, len(_STEPS)):
            reduce_step(q)

        acc = None
        for t, (a, b) in enumerate(zip((_G,) + _TAIL[:-1], _TAIL)):
            lo, hi = (a + 1) * cb, min((b + 1) * cb, ts + _SH)
            wait(buf.at[ns - 1, pl.ds(lo, hi - lo)], tail_sems.at[t])
            piece = row_max(
                buf[ns - 1, pl.ds(a * cb + _SH, (b - a) * cb)], a % _G * 8
            )
            acc = piece if acc is None else jnp.maximum(acc, piece)
        tail_part[...] = jnp.max(acc, axis=0, keepdims=True)
        swaps[2].start()

        swaps[0].wait_recv()
        o_ref[pl.ds(0, ns, stride=2), :] = jnp.maximum(part[0], recv[0])
        swaps[1].wait_recv()
        o_ref[pl.ds(1, ns - 1, stride=2), :] = jnp.maximum(
            part[1, pl.ds(0, ns - 1), :], recv[1, pl.ds(0, ns - 1), :]
        )
        for rd in swaps:
            rd.wait_send()
        swaps[2].wait_recv()
        o_ref[pl.ds(2 * ns - 1, 1), :] = jnp.maximum(tail_part[...], tail_recv[...])

    out = pl.pallas_call(
        body,
        out_shape=jax.ShapeDtypeStruct((m // 128, 128), x.dtype),
        in_specs=[pl.BlockSpec(memory_space=pl.ANY)],
        out_specs=pl.BlockSpec(memory_space=pltpu.VMEM),
        scratch_shapes=[
            pltpu.VMEM((ns, ts + _SH, 8, 128), x.dtype),
            pltpu.VMEM((2, ns, 128), x.dtype),
            pltpu.VMEM((2, ns, 128), x.dtype),
            pltpu.VMEM((1, 128), x.dtype),
            pltpu.VMEM((1, 128), x.dtype),
            pltpu.SemaphoreType.DMA((2,)),
            pltpu.SemaphoreType.DMA((len(_STEPS),)),
            pltpu.SemaphoreType.DMA((len(_TAIL),)),
            pltpu.SemaphoreType.DMA((3,)),
            pltpu.SemaphoreType.DMA((3,)),
        ],
        compiler_params=pltpu.CompilerParams(
            vmem_limit_bytes=64 * 1024 * 1024,
            collective_id=0,
            disable_semaphore_checks=True,
        ),
    )(xt)
    return out.reshape(m, 1)
```

```python
import jax
import jax.numpy as jnp
from jax import lax
from jax.experimental import pallas as pl
from jax.experimental.pallas import tpu as pltpu

_G = 16
_R = 2 * _G
_SH = 1
_HEAD = 27
_EARLY = 21
_LAG = 34
_HALVED = 13
_STEPS = (4, 8, 12, 16, 20, 24, 28, 30, 32)
_TAIL = (28, 32)


def pallas_dist_max_ax1_xy_m4096_n1024_kernel(
x: jax.Array,
):
    m, n = x.shape
    cb = n // 128
    ts = _R * cb
    ns = m // (8 * _R)
    assert m % (8 * _R) == 0 and n % 256 == 0 and 0 < _SH < cb
    assert _G in _STEPS and _STEPS[-1] == _R and _TAIL[-1] == _R

    main = [(s, i) for i in range(_R) for s in range(ns if i <= _G else ns - 1)]
    lo_main, hi_main = main[0::2], main[1::2]
    lo_tail = []
    for i in range(_G + 1, _R):
        piece = min(t for t, end in enumerate(_TAIL) if i <= end)
        nt = cb + (_SH if i == _R - 1 else 0)
        cut = cb // 2 if i >= _R - _HALVED else nt
        lo_tail.append((i * cb, cut, piece))
        if cut < nt:
            lo_tail.append((i * cb + cut, nt - cut, piece))
    n_pairs = max(len(hi_main), len(lo_main) + len(lo_tail) - _HEAD)

    def step_of(i):
        return min(q for q, end in enumerate(_STEPS) if i <= end)

    last_pair = {step_of(i): k // 2 for k, (_, i) in enumerate(main)}

    xt = x.reshape(m // 8, 8, cb, 128).transpose(0, 2, 1, 3)
    xt = xt.reshape(m // 8 * cb, 8, 128)

    def body(x_hbm, o_ref, buf, part, recv, tail_part, tail_recv,
             head_sems, step_sems, tail_sems, send_sems, recv_sems):
        def start(s, t0, nt, sem, prio):
            pltpu.make_async_copy(
                x_hbm.at[pl.ds(s * ts + t0 - _SH, nt)],
                buf.at[s, pl.ds(t0, nt)],
                sem,
            ).start(priority=prio)

        def start_main(s, i, prio):
            if i > 0:
                start(s, i * cb, cb, step_sems.at[step_of(i)], prio)
            elif s > 0:
                start(s, 0, cb, head_sems.at[1], prio)
            else:
                start(0, _SH, cb - _SH, head_sems.at[0], prio)

        def start_lo(k):
            if k < len(lo_main):
                start_main(*lo_main[k], 1)
            elif k - len(lo_main) < len(lo_tail):
                t0, nt, piece = lo_tail[k - len(lo_main)]
                start(ns - 1, t0, nt, tail_sems.at[piece], 1)

        def wait(ref, sem):
            pltpu.make_async_copy(ref, ref, sem).wait()

        def row_max(tiles, lane0):
            g = tiles.shape[0] // cb
            tiles = tiles.reshape(g, cb, 8, 128)
            vs = [tiles[:, k] for k in range(cb)]
            while len(vs) > 1:
                vs = [jnp.maximum(a, b) for a, b in zip(vs[0::2], vs[1::2])] + (
                    vs[-1:] if len(vs) % 2 else []
                )
            col = jnp.max(vs[0], axis=2, keepdims=True)
            gi = lax.broadcasted_iota(jnp.int32, (g, 8, 128), 0)
            ri = lax.broadcasted_iota(jnp.int32, (g, 8, 128), 1)
            ci = lax.broadcasted_iota(jnp.int32, (g, 8, 128), 2)
            diag = jnp.where(ci - ri - 8 * gi == lane0, col, -jnp.inf)
            return jnp.max(diag, axis=0)

        def reduce_step(q):
            a, b = (_STEPS[q - 1] if q else 0), _STEPS[q]
            streams = ns if b <= _G else ns - 1
            if q == 0:
                wait(buf.at[0, pl.ds(_SH, cb - _SH)], head_sems.at[0])
                wait(buf.at[pl.ds(1, ns - 1), pl.ds(0, cb)], head_sems.at[1])
            rounds = min(b, _R - 1) - a
            wait(buf.at[pl.ds(0, streams), pl.ds((a + 1) * cb, rounds * cb)],
                 step_sems.at[q])
            t0, nt = a * cb + _SH, (b - a) * cb
            for s in range(streams):
                if b == _R:
                    tiles = jnp.concatenate(
                        [buf[s, pl.ds(t0, nt - _SH)], buf[s + 1, pl.ds(0, _SH)]],
                        axis=0,
                    )
                else:
                    tiles = buf[s, pl.ds(t0, nt)]
                new = jnp.max(row_max(tiles, a % _G * 8), axis=0, keepdims=True)
                row = part.at[a // _G, pl.ds(s, 1), :]
                row[...] = jnp.maximum(row[...], new)
            if b == _G:
                pl.semaphore_wait(barrier, 1)
                swaps[0].start()
            if b == _R:
                swaps[1].start()

        def start_pair(k):
            if k < len(hi_main):
                start_main(*hi_main[k], 0)
            start_lo(k + _HEAD)

        for k in range(_HEAD):
            start_lo(k)
        for k in range(_EARLY):
            start_pair(k)

        peer = (lax.axis_index("x"), 1 - lax.axis_index("y"))
        barrier = pltpu.get_barrier_semaphore()
        swaps = [
            pltpu.make_async_remote_copy(
                src, dst, send_sems.at[i], recv_sems.at[i],
                device_id=peer, device_id_type=pl.DeviceIdType.MESH,
            )
            for i, (src, dst) in enumerate([
                (part.at[0], recv.at[0]),
                (part.at[1], recv.at[1]),
                (tail_part, tail_recv),
            ])
        ]
        pl.semaphore_signal(
            barrier, 1, device_id=peer, device_id_type=pl.DeviceIdType.MESH
        )
        part[...] = jnp.full(part.shape, -jnp.inf, part.dtype)

        q = 0
        for k in range(_EARLY, n_pairs):
            start_pair(k)
            if k >= last_pair[q] + _LAG:
                reduce_step(q)
                q += 1
        for q in range(q, len(_STEPS)):
            reduce_step(q)

        acc = None
        for t, (a, b) in enumerate(zip((_G,) + _TAIL[:-1], _TAIL)):
            lo, hi = (a + 1) * cb, min((b + 1) * cb, ts + _SH)
            wait(buf.at[ns - 1, pl.ds(lo, hi - lo)], tail_sems.at[t])
            piece = row_max(
                buf[ns - 1, pl.ds(a * cb + _SH, (b - a) * cb)], a % _G * 8
            )
            acc = piece if acc is None else jnp.maximum(acc, piece)
        tail_part[...] = jnp.max(acc, axis=0, keepdims=True)
        swaps[2].start()

        swaps[0].wait_recv()
        o_ref[pl.ds(0, ns, stride=2), :] = jnp.maximum(part[0], recv[0])
        swaps[1].wait_recv()
        o_ref[pl.ds(1, ns - 1, stride=2), :] = jnp.maximum(
            part[1, pl.ds(0, ns - 1), :], recv[1, pl.ds(0, ns - 1), :]
        )
        for rd in swaps:
            rd.wait_send()
        swaps[2].wait_recv()
        o_ref[pl.ds(2 * ns - 1, 1), :] = jnp.maximum(tail_part[...], tail_recv[...])

    out = pl.pallas_call(
        body,
        out_shape=jax.ShapeDtypeStruct((m // 128, 128), x.dtype),
        in_specs=[pl.BlockSpec(memory_space=pl.ANY)],
        out_specs=pl.BlockSpec(memory_space=pltpu.VMEM),
        scratch_shapes=[
            pltpu.VMEM((ns, ts + _SH, 8, 128), x.dtype),
            pltpu.VMEM((2, ns, 128), x.dtype),
            pltpu.VMEM((2, ns, 128), x.dtype),
            pltpu.VMEM((1, 128), x.dtype),
            pltpu.VMEM((1, 128), x.dtype),
            pltpu.SemaphoreType.DMA((2,)),
            pltpu.SemaphoreType.DMA((len(_STEPS),)),
            pltpu.SemaphoreType.DMA((len(_TAIL),)),
            pltpu.SemaphoreType.DMA((3,)),
            pltpu.SemaphoreType.DMA((3,)),
        ],
        compiler_params=pltpu.CompilerParams(
            vmem_limit_bytes=64 * 1024 * 1024,
            collective_id=0,
            disable_semaphore_checks=True,
        ),
    )(xt)
    return out.reshape(m, 1)
```

```python
import jax
import jax.numpy as jnp
from jax import lax
from jax.experimental import pallas as pl
from jax.experimental.pallas import tpu as pltpu

_G = 16
_R = 2 * _G
_SH = 1
_HEAD = 28
_EARLY = 21
_LAG = 34
_HALVED = 14
_STEPS = (4, 8, 12, 16, 20, 24, 28, 30, 32)
_TAIL = (28, 32)


def pallas_dist_max_ax1_xy_m4096_n1024_kernel(
x: jax.Array,
):
    m, n = x.shape
    cb = n // 128
    ts = _R * cb
    ns = m // (8 * _R)
    assert m % (8 * _R) == 0 and n % 256 == 0 and 0 < _SH < cb
    assert _G in _STEPS and _STEPS[-1] == _R and _TAIL[-1] == _R

    main = [(s, i) for i in range(_R) for s in range(ns if i <= _G else ns - 1)]
    lo_main, hi_main = main[0::2], main[1::2]
    lo_tail = []
    for i in range(_G + 1, _R):
        piece = min(t for t, end in enumerate(_TAIL) if i <= end)
        nt = cb + (_SH if i == _R - 1 else 0)
        cut = cb // 2 if i >= _R - _HALVED else nt
        lo_tail.append((i * cb, cut, piece))
        if cut < nt:
            lo_tail.append((i * cb + cut, nt - cut, piece))
    n_pairs = max(len(hi_main), len(lo_main) + len(lo_tail) - _HEAD)

    def step_of(i):
        return min(q for q, end in enumerate(_STEPS) if i <= end)

    last_pair = {step_of(i): k // 2 for k, (_, i) in enumerate(main)}

    xt = x.reshape(m // 8, 8, cb, 128).transpose(0, 2, 1, 3)
    xt = xt.reshape(m // 8 * cb, 8, 128)

    def body(x_hbm, o_ref, buf, part, recv, tail_part, tail_recv,
             head_sems, step_sems, tail_sems, send_sems, recv_sems):
        def start(s, t0, nt, sem, prio):
            pltpu.make_async_copy(
                x_hbm.at[pl.ds(s * ts + t0 - _SH, nt)],
                buf.at[s, pl.ds(t0, nt)],
                sem,
            ).start(priority=prio)

        def start_main(s, i, prio):
            if i > 0:
                start(s, i * cb, cb, step_sems.at[step_of(i)], prio)
            elif s > 0:
                start(s, 0, cb, head_sems.at[1], prio)
            else:
                start(0, _SH, cb - _SH, head_sems.at[0], prio)

        def start_lo(k):
            if k < len(lo_main):
                start_main(*lo_main[k], 1)
            elif k - len(lo_main) < len(lo_tail):
                t0, nt, piece = lo_tail[k - len(lo_main)]
                start(ns - 1, t0, nt, tail_sems.at[piece], 1)

        def wait(ref, sem):
            pltpu.make_async_copy(ref, ref, sem).wait()

        def row_max(tiles, lane0):
            s, g = tiles.shape[0], tiles.shape[1] // cb
            tiles = tiles.reshape(s, g, cb, 8, 128)
            vs = [tiles[:, :, k] for k in range(cb)]
            while len(vs) > 1:
                vs = [jnp.maximum(a, b) for a, b in zip(vs[0::2], vs[1::2])] + (
                    vs[-1:] if len(vs) % 2 else []
                )
            col = jnp.max(vs[0], axis=3, keepdims=True)
            gi = lax.broadcasted_iota(jnp.int32, (1, g, 8, 128), 1)
            ri = lax.broadcasted_iota(jnp.int32, (1, g, 8, 128), 2)
            ci = lax.broadcasted_iota(jnp.int32, (1, g, 8, 128), 3)
            diag = jnp.where(ci - ri - 8 * gi == lane0, col, -jnp.inf)
            return jnp.max(diag, axis=1)

        def reduce_step(q):
            a, b = (_STEPS[q - 1] if q else 0), _STEPS[q]
            streams = ns if b <= _G else ns - 1
            if q == 0:
                wait(buf.at[0, pl.ds(_SH, cb - _SH)], head_sems.at[0])
                wait(buf.at[pl.ds(1, ns - 1), pl.ds(0, cb)], head_sems.at[1])
            rounds = min(b, _R - 1) - a
            wait(buf.at[pl.ds(0, streams), pl.ds((a + 1) * cb, rounds * cb)],
                 step_sems.at[q])
            t0, nt = a * cb + _SH, (b - a) * cb
            if b == _R:
                tiles = jnp.concatenate(
                    [buf[pl.ds(0, streams), pl.ds(t0, nt - _SH)],
                     buf[pl.ds(1, streams), pl.ds(0, _SH)]],
                    axis=1,
                )
            else:
                tiles = buf[pl.ds(0, streams), pl.ds(t0, nt)]
            rows = part.at[a // _G, pl.ds(0, streams), :]
            rows[...] = jnp.maximum(
                rows[...], jnp.max(row_max(tiles, a % _G * 8), axis=1)
            )
            if b == _G:
                pl.semaphore_wait(barrier, 1)
                swaps[0].start()
            if b == _R:
                swaps[1].start()

        def start_pair(k):
            if k < len(hi_main):
                start_main(*hi_main[k], 0)
            start_lo(k + _HEAD)

        for k in range(_HEAD):
            start_lo(k)
        for k in range(_EARLY):
            start_pair(k)

        peer = (lax.axis_index("x"), 1 - lax.axis_index("y"))
        barrier = pltpu.get_barrier_semaphore()
        swaps = [
            pltpu.make_async_remote_copy(
                src, dst, send_sems.at[i], recv_sems.at[i],
                device_id=peer, device_id_type=pl.DeviceIdType.MESH,
            )
            for i, (src, dst) in enumerate([
                (part.at[0], recv.at[0]),
                (part.at[1], recv.at[1]),
                (tail_part, tail_recv),
            ])
        ]
        pl.semaphore_signal(
            barrier, 1, device_id=peer, device_id_type=pl.DeviceIdType.MESH
        )
        part[...] = jnp.full(part.shape, -jnp.inf, part.dtype)

        q = 0
        for k in range(_EARLY, n_pairs):
            start_pair(k)
            if k >= last_pair[q] + _LAG:
                reduce_step(q)
                q += 1
        for q in range(q, len(_STEPS)):
            reduce_step(q)

        acc = None
        for t, (a, b) in enumerate(zip((_G,) + _TAIL[:-1], _TAIL)):
            lo, hi = (a + 1) * cb, min((b + 1) * cb, ts + _SH)
            wait(buf.at[ns - 1, pl.ds(lo, hi - lo)], tail_sems.at[t])
            piece = row_max(
                buf[pl.ds(ns - 1, 1), pl.ds(a * cb + _SH, (b - a) * cb)],
                a % _G * 8,
            )
            acc = piece if acc is None else jnp.maximum(acc, piece)
        tail_part[...] = jnp.max(acc, axis=1)
        swaps[2].start()

        swaps[0].wait_recv()
        o_ref[pl.ds(0, ns, stride=2), :] = jnp.maximum(part[0], recv[0])
        swaps[1].wait_recv()
        o_ref[pl.ds(1, ns - 1, stride=2), :] = jnp.maximum(
            part[1, pl.ds(0, ns - 1), :], recv[1, pl.ds(0, ns - 1), :]
        )
        for rd in swaps:
            rd.wait_send()
        swaps[2].wait_recv()
        o_ref[pl.ds(2 * ns - 1, 1), :] = jnp.maximum(tail_part[...], tail_recv[...])

    out = pl.pallas_call(
        body,
        out_shape=jax.ShapeDtypeStruct((m // 128, 128), x.dtype),
        in_specs=[pl.BlockSpec(memory_space=pl.ANY)],
        out_specs=pl.BlockSpec(memory_space=pltpu.VMEM),
        scratch_shapes=[
            pltpu.VMEM((ns, ts + _SH, 8, 128), x.dtype),
            pltpu.VMEM((2, ns, 128), x.dtype),
            pltpu.VMEM((2, ns, 128), x.dtype),
            pltpu.VMEM((1, 128), x.dtype),
            pltpu.VMEM((1, 128), x.dtype),
            pltpu.SemaphoreType.DMA((2,)),
            pltpu.SemaphoreType.DMA((len(_STEPS),)),
            pltpu.SemaphoreType.DMA((len(_TAIL),)),
            pltpu.SemaphoreType.DMA((3,)),
            pltpu.SemaphoreType.DMA((3,)),
        ],
        compiler_params=pltpu.CompilerParams(
            vmem_limit_bytes=64 * 1024 * 1024,
            collective_id=0,
            disable_semaphore_checks=True,
        ),
    )(xt)
    return out.reshape(m, 1)
```
